```python
import numpy as np

kernel_name = "dist_argmax_global_i_m4096_n1024"

def setup_inputs():
    return {"x": np.random.randn(16384, 1024).astype(np.float32)}

def reference(x: np.ndarray) -> np.ndarray:
    idx = np.argmax(x, axis=0).astype(np.float32)
    val = np.max(x, axis=0)
    return np.stack([val, idx], axis=0)
```

```python
import functools

import jax
import jax.numpy as jnp
from jax import lax
from jax.experimental import pallas as pl
from jax.experimental.pallas import tpu as pltpu

N_DEV = 4
CHUNK = 512
IN_FLIGHT = 3
UNROLL = 8


def pallas_dist_argmax_global_i_m4096_n1024_kernel(
x: jax.Array,
):
    m_per, n = x.shape
    n_chunks = m_per // CHUNK
    assert n_chunks * CHUNK == m_per

    def body(x_hbm, out_ref, buf, comm, sems, send_sems, recv_sems):
        my = lax.axis_index("i")

        barrier = pltpu.get_barrier_semaphore()
        for d in range(1, N_DEV):
            pl.semaphore_signal(
                barrier, inc=1, device_id=((my + d) % N_DEV,),
                device_id_type=pl.DeviceIdType.MESH)

        def chunk_copy(c):
            return pltpu.make_async_copy(
                x_hbm.at[pl.ds(c * CHUNK, CHUNK)],
                buf.at[pl.ds(c * CHUNK, CHUNK)],
                sems.at[c])

        for c in range(min(IN_FLIGHT, n_chunks)):
            chunk_copy(c).start()

        m = jnp.full((8, n), -jnp.inf, jnp.float32)
        ix = jnp.zeros((8, n), jnp.int32)
        for c in range(n_chunks):
            chunk_copy(c).wait()
            if c + IN_FLIGHT < n_chunks:
                chunk_copy(c + IN_FLIGHT).start()

            def step(j, carry, c=c):
                m, ix = carry
                r = c * (CHUNK // 8) + j
                v = buf[pl.ds(pl.multiple_of(r * 8, 8), 8), :]
                take = jnp.logical_and(
                    jnp.logical_or(v > m, v != v), m == m)
                return jnp.where(take, v, m), jnp.where(take, r, ix)

            m, ix = lax.fori_loop(0, CHUNK // 8, step, (m, ix), unroll=UNROLL)

        big = jnp.int32(2 ** 30)
        row = ix * 8 + lax.broadcasted_iota(jnp.int32, (8, n), 0)
        cmax = jnp.max(m, axis=0, keepdims=True)
        hit = jnp.logical_or(m == cmax, m != m)
        cidx = jnp.min(jnp.where(hit, row, big), axis=0, keepdims=True)
        cidx = cidx + my * m_per
        comm[my, 0:1, :] = cmax
        comm[my, 1:2, :] = cidx.astype(jnp.float32)

        pl.semaphore_wait(barrier, N_DEV - 1)
        rdmas = []
        for d in range(1, N_DEV):
            rdma = pltpu.make_async_remote_copy(
                src_ref=comm.at[my], dst_ref=comm.at[my],
                send_sem=send_sems.at[d - 1], recv_sem=recv_sems.at[d - 1],
                device_id=((my + d) % N_DEV,),
                device_id_type=pl.DeviceIdType.MESH)
            rdma.start()
            rdmas.append(rdma)
        for rdma in rdmas:
            rdma.wait()

        vals = comm[:, 0, :]
        idxs = comm[:, 1, :]
        gmax = jnp.max(vals, axis=0, keepdims=True)
        ghit = jnp.logical_or(vals == gmax, vals != vals)
        gidx = jnp.min(jnp.where(ghit, idxs, jnp.float32(2 ** 30)),
                       axis=0, keepdims=True)
        out_ref[0:1, :] = gmax
        out_ref[1:2, :] = gidx

    return pl.pallas_call(
        body,
        out_shape=jax.ShapeDtypeStruct((2, n), jnp.float32),
        in_specs=[pl.BlockSpec(memory_space=pl.ANY)],
        out_specs=pl.BlockSpec(memory_space=pltpu.VMEM),
        scratch_shapes=[
            pltpu.VMEM((m_per, n), jnp.float32),
            pltpu.VMEM((N_DEV, 2, n), jnp.float32),
            pltpu.SemaphoreType.DMA((n_chunks,)),
            pltpu.SemaphoreType.DMA((N_DEV - 1,)),
            pltpu.SemaphoreType.DMA((N_DEV - 1,)),
        ],
        compiler_params=pltpu.CompilerParams(
            collective_id=0, vmem_limit_bytes=64 * 1024 * 1024),
    )(x)
```

```python
import jax
import jax.numpy as jnp
from jax import lax
from jax.experimental import pallas as pl
from jax.experimental.pallas import tpu as pltpu

N_DEV = 4
SIZES = (512,) * 7 + (256, 128, 64, 64)
IN_FLIGHT = 3
UNROLL = 8


def pallas_dist_argmax_global_i_m4096_n1024_kernel(
x: jax.Array,
):
    m_per, n = x.shape
    n_chunks = len(SIZES)
    assert sum(SIZES) == m_per
    offs = [sum(SIZES[:i]) for i in range(n_chunks)]

    def body(x_hbm, out_ref, buf, comm, sems, send_sems, recv_sems):
        my = lax.axis_index("i")

        barrier = pltpu.get_barrier_semaphore()
        for d in range(1, N_DEV):
            pl.semaphore_signal(
                barrier, inc=1, device_id=((my + d) % N_DEV,),
                device_id_type=pl.DeviceIdType.MESH)

        def chunk_copy(c):
            return pltpu.make_async_copy(
                x_hbm.at[pl.ds(offs[c], SIZES[c])],
                buf.at[pl.ds(offs[c], SIZES[c])],
                sems.at[c])

        for c in range(min(IN_FLIGHT, n_chunks)):
            chunk_copy(c).start()

        m = jnp.full((8, n), -jnp.inf, jnp.float32)
        ix = jnp.zeros((8, n), jnp.int32)
        for c in range(n_chunks):
            chunk_copy(c).wait()
            if c + IN_FLIGHT < n_chunks:
                chunk_copy(c + IN_FLIGHT).start()

            def step(j, carry, c=c):
                m, ix = carry
                r = offs[c] // 8 + j
                v = buf[pl.ds(pl.multiple_of(r * 8, 8), 8), :]
                take = jnp.logical_and(
                    jnp.logical_or(v > m, v != v), m == m)
                return jnp.where(take, v, m), jnp.where(take, r, ix)

            m, ix = lax.fori_loop(0, SIZES[c] // 8, step, (m, ix), unroll=UNROLL)

        big = jnp.int32(2 ** 30)
        row = ix * 8 + lax.broadcasted_iota(jnp.int32, (8, n), 0)
        cmax = jnp.max(m, axis=0, keepdims=True)
        hit = jnp.logical_or(m == cmax, m != m)
        cidx = jnp.min(jnp.where(hit, row, big), axis=0, keepdims=True)
        cidx = cidx + my * m_per
        comm[my, 0:1, :] = cmax
        comm[my, 1:2, :] = cidx.astype(jnp.float32)

        pl.semaphore_wait(barrier, N_DEV - 1)
        rdmas = []
        for d in range(1, N_DEV):
            rdma = pltpu.make_async_remote_copy(
                src_ref=comm.at[my], dst_ref=comm.at[my],
                send_sem=send_sems.at[d - 1], recv_sem=recv_sems.at[d - 1],
                device_id=((my + d) % N_DEV,),
                device_id_type=pl.DeviceIdType.MESH)
            rdma.start()
            rdmas.append(rdma)
        for rdma in rdmas:
            rdma.wait()

        vals = comm[:, 0, :]
        idxs = comm[:, 1, :]
        gmax = jnp.max(vals, axis=0, keepdims=True)
        ghit = jnp.logical_or(vals == gmax, vals != vals)
        gidx = jnp.min(jnp.where(ghit, idxs, jnp.float32(2 ** 30)),
                       axis=0, keepdims=True)
        out_ref[0:1, :] = gmax
        out_ref[1:2, :] = gidx

    return pl.pallas_call(
        body,
        out_shape=jax.ShapeDtypeStruct((2, n), jnp.float32),
        in_specs=[pl.BlockSpec(memory_space=pl.ANY)],
        out_specs=pl.BlockSpec(memory_space=pltpu.VMEM),
        scratch_shapes=[
            pltpu.VMEM((m_per, n), jnp.float32),
            pltpu.VMEM((N_DEV, 2, n), jnp.float32),
            pltpu.SemaphoreType.DMA((n_chunks,)),
            pltpu.SemaphoreType.DMA((N_DEV - 1,)),
            pltpu.SemaphoreType.DMA((N_DEV - 1,)),
        ],
        compiler_params=pltpu.CompilerParams(
            collective_id=0, vmem_limit_bytes=64 * 1024 * 1024),
    )(x)
```
